```python
import numpy as np

kernel_name = "dist_mean_ax0_shard0_i_m2048_n1024"

def setup_inputs():
    return {"x": np.random.randn(8192, 1024).astype(np.float32)}

def reference(x: np.ndarray) -> np.ndarray:
    return np.mean(x, axis=0, keepdims=True)
```

```python
import jax
import jax.numpy as jnp
from jax import lax
from jax.experimental import pallas as pl
from jax.experimental.pallas import tpu as pltpu

N_DEV = 4
SUBLANES = 8


def pallas_dist_mean_ax0_shard0_i_m2048_n1024_kernel(
x: jax.Array,
):
    m_per, n = x.shape
    chunk_rows = [256] * 8
    assert sum(chunk_rows) == m_per
    n_chunks = len(chunk_rows)
    offsets = [sum(chunk_rows[:c]) for c in range(n_chunks)]
    inv_count = 1.0 / float(N_DEV * m_per)

    def body(x_hbm, out_hbm, buf, comm, out_vmem, load_sems, send_sems, recv_sems, out_sem):
        my = lax.axis_index("i")

        loads = [
            pltpu.make_async_copy(
                x_hbm.at[pl.ds(offsets[c], chunk_rows[c])],
                buf.at[pl.ds(offsets[c], chunk_rows[c])],
                load_sems.at[c],
            )
            for c in range(n_chunks)
        ]
        for cp in loads:
            cp.start()

        barrier = pltpu.get_barrier_semaphore()
        for d in range(1, N_DEV):
            pl.semaphore_signal(
                barrier, inc=1,
                device_id=((my + d) % N_DEV,),
                device_id_type=pl.DeviceIdType.MESH,
            )

        acc = jnp.zeros((SUBLANES, n), jnp.float32)
        for c in range(n_chunks):
            loads[c].wait()
            blk = buf[pl.ds(offsets[c], chunk_rows[c]), :]
            acc = acc + jnp.sum(blk.reshape(chunk_rows[c] // SUBLANES, SUBLANES, n), axis=0)
        comm[my] = jnp.sum(acc, axis=0, keepdims=True)

        pl.semaphore_wait(barrier, N_DEV - 1)

        sends = []
        for d in range(1, N_DEV):
            rdma = pltpu.make_async_remote_copy(
                src_ref=comm.at[my],
                dst_ref=comm.at[my],
                send_sem=send_sems.at[d - 1],
                recv_sem=recv_sems.at[d - 1],
                device_id=((my + d) % N_DEV,),
                device_id_type=pl.DeviceIdType.MESH,
            )
            rdma.start()
            sends.append(rdma)
        for d in range(1, N_DEV):
            src = (my + N_DEV - d) % N_DEV
            pltpu.make_async_remote_copy(
                src_ref=comm.at[src],
                dst_ref=comm.at[src],
                send_sem=send_sems.at[d - 1],
                recv_sem=recv_sems.at[d - 1],
                device_id=(src,),
                device_id_type=pl.DeviceIdType.MESH,
            ).wait_recv()

        total = (comm[0] + comm[1]) + (comm[2] + comm[3])
        out_vmem[...] = total * inv_count
        wb = pltpu.make_async_copy(out_vmem, out_hbm, out_sem)
        wb.start()
        for rdma in sends:
            rdma.wait_send()
        wb.wait()

    return pl.pallas_call(
        body,
        out_shape=jax.ShapeDtypeStruct((1, n), jnp.float32),
        in_specs=[pl.BlockSpec(memory_space=pl.ANY)],
        out_specs=pl.BlockSpec(memory_space=pl.ANY),
        scratch_shapes=[
            pltpu.VMEM((m_per, n), jnp.float32),
            pltpu.VMEM((N_DEV, 1, n), jnp.float32),
            pltpu.VMEM((1, n), jnp.float32),
            pltpu.SemaphoreType.DMA((n_chunks,)),
            pltpu.SemaphoreType.DMA((N_DEV - 1,)),
            pltpu.SemaphoreType.DMA((N_DEV - 1,)),
            pltpu.SemaphoreType.DMA,
        ],
        compiler_params=pltpu.CompilerParams(collective_id=0, vmem_limit_bytes=32 * 1024 * 1024),
    )(x)
```

```python
import jax
import jax.numpy as jnp
from jax import lax
from jax.experimental import pallas as pl
from jax.experimental.pallas import tpu as pltpu

_N_DEV = 4
_SUB = 8
_LATE = 2
_OFF_ROWS = 104
_TAIL_ROWS = 192
_TAIL_COLS = 128
_MESH = pl.DeviceIdType.MESH


def _colsum8(blk):
    r, c = blk.shape
    return jnp.sum(blk.reshape(r // _SUB, _SUB, c), axis=0)


def pallas_dist_mean_ax0_shard0_i_m2048_n1024_kernel(
x: jax.Array,
):
    m_per, n = x.shape
    head = 2 * _OFF_ROWS
    t0 = m_per - _TAIL_ROWS
    n_a = n - _TAIL_COLS
    chunk_rows = [head, 512, 512, t0 - head - 1024 - 128, 128]
    assert min(chunk_rows) > 0 and all(r % _SUB == 0 for r in chunk_rows)
    assert sum(chunk_rows) == t0 and n % 128 == 0 and n_a > 0
    n_chunks = len(chunk_rows)
    offsets = [sum(chunk_rows[:c]) for c in range(n_chunks)]
    inv_count = 1.0 / float(_N_DEV * m_per)

    msg_diag_a = (2, 0, n_a, 0)
    msg_diag_b = (2, n_a, _TAIL_COLS, 1)
    msg_right = (1, 0, n, 2)
    msg_left = (3, 0, n, 3)

    def body(x_hbm, out_ref, buf, obuf, comm,
             load_sems, send_sems, recv_sems, osend_sems, orecv_sem):
        my = lax.axis_index("i")

        loads = [
            pltpu.make_async_copy(
                x_hbm.at[pl.ds(offsets[c], chunk_rows[c])],
                buf.at[pl.ds(offsets[c], chunk_rows[c])],
                load_sems.at[c],
            )
            for c in range(n_chunks)
        ]
        tail_a = pltpu.make_async_copy(
            x_hbm.at[pl.ds(t0, _TAIL_ROWS), pl.ds(0, n_a)],
            buf.at[pl.ds(t0, _TAIL_ROWS), pl.ds(0, n_a)],
            load_sems.at[n_chunks],
        )
        tail_b = pltpu.make_async_copy(
            x_hbm.at[pl.ds(t0, _TAIL_ROWS), pl.ds(n_a, _TAIL_COLS)],
            buf.at[pl.ds(t0, _TAIL_ROWS), pl.ds(n_a, _TAIL_COLS)],
            load_sems.at[n_chunks + 1],
        )

        @pl.when(my != _LATE)
        def _():
            loads[0].start()

        for cp in loads[1:]:
            cp.start()
        tail_a.start()
        tail_b.start()

        barrier = pltpu.get_barrier_semaphore()
        for d in range(1, _N_DEV):
            pl.semaphore_signal(
                barrier, inc=1, device_id=((my + d) % _N_DEV,), device_id_type=_MESH
            )
        pl.semaphore_wait(barrier, _N_DEV - 1)

        def offload(j):
            return pltpu.make_async_remote_copy(
                src_ref=x_hbm.at[pl.ds(j * _OFF_ROWS, _OFF_ROWS)],
                dst_ref=obuf,
                send_sem=osend_sems.at[j],
                recv_sem=orecv_sem,
                device_id=((_LATE + (1 if j else _N_DEV - 1)) % _N_DEV,),
                device_id_type=_MESH,
            )

        @pl.when(my == _LATE)
        def _():
            offload(0).start()
            offload(1).start()

        def zeros():
            return jnp.zeros((_SUB, n), jnp.float32)

        def own_head():
            loads[0].wait()
            return _colsum8(buf[pl.ds(0, head), :])

        def shipped_rows():
            offload(0).wait_recv()
            return _colsum8(obuf[...])

        acc = lax.cond(my != _LATE, own_head, zeros)
        for c in range(1, n_chunks):
            loads[c].wait()
            acc = acc + _colsum8(buf[pl.ds(offsets[c], chunk_rows[c]), :])
        acc = acc + lax.cond((my % 2) != (_LATE % 2), shipped_rows, zeros)

        def message(spec, owner):
            dist, c0, width, slot = spec
            part = comm.at[owner, :, pl.ds(c0, width)]
            return pltpu.make_async_remote_copy(
                src_ref=part,
                dst_ref=part,
                send_sem=send_sems.at[slot],
                recv_sem=recv_sems.at[slot],
                device_id=((my + dist) % _N_DEV,),
                device_id_type=_MESH,
            )

        tail_a.wait()
        a = acc[:, :n_a] + _colsum8(buf[pl.ds(t0, _TAIL_ROWS), pl.ds(0, n_a)])
        comm[my, :, pl.ds(0, n_a)] = jnp.sum(a, axis=0, keepdims=True)
        message(msg_diag_a, my).start()

        tail_b.wait()
        b = acc[:, n_a:] + _colsum8(
            buf[pl.ds(t0, _TAIL_ROWS), pl.ds(n_a, _TAIL_COLS)]
        )
        comm[my, :, pl.ds(n_a, _TAIL_COLS)] = jnp.sum(b, axis=0, keepdims=True)
        for spec in (msg_diag_b, msg_right, msg_left):
            message(spec, my).start()

        for spec in (msg_diag_a, msg_diag_b, msg_right, msg_left):
            message(spec, my).wait_send()

        @pl.when(my == _LATE)
        def _():
            offload(0).wait_send()
            offload(1).wait_send()

        for spec in (msg_right, msg_left, msg_diag_a, msg_diag_b):
            sender = (my + _N_DEV - spec[0]) % _N_DEV
            message(spec, sender).wait_recv()

        total = (comm[0] + comm[1]) + (comm[2] + comm[3])
        out_ref[...] = total * inv_count

    return pl.pallas_call(
        body,
        out_shape=jax.ShapeDtypeStruct((1, n), jnp.float32),
        in_specs=[pl.BlockSpec(memory_space=pl.ANY)],
        out_specs=pl.BlockSpec(memory_space=pltpu.VMEM),
        scratch_shapes=[
            pltpu.VMEM((m_per, n), jnp.float32),
            pltpu.VMEM((_OFF_ROWS, n), jnp.float32),
            pltpu.VMEM((_N_DEV, 1, n), jnp.float32),
            pltpu.SemaphoreType.DMA((n_chunks + 2,)),
            pltpu.SemaphoreType.DMA((4,)),
            pltpu.SemaphoreType.DMA((4,)),
            pltpu.SemaphoreType.DMA((2,)),
            pltpu.SemaphoreType.DMA,
        ],
        compiler_params=pltpu.CompilerParams(
            collective_id=0,
            vmem_limit_bytes=32 * 1024 * 1024,
            disable_semaphore_checks=True,
            disable_bounds_checks=True,
        ),
    )(x)
```

```python
import jax
import jax.numpy as jnp
from jax import lax
from jax.experimental import pallas as pl
from jax.experimental.pallas import tpu as pltpu

_N_DEV = 4
_SUB = 8
_LATE = 2
_OFF_ROWS = 104
_TAIL_A_ROWS = (128, 32)
_TAIL_COLS = 128
_MESH = pl.DeviceIdType.MESH


def _colsum8(blk):
    r, c = blk.shape
    return jnp.sum(blk.reshape(r // _SUB, _SUB, c), axis=0)


def _treesum8(blk):
    parts = [blk[i:i + _SUB, :] for i in range(0, blk.shape[0], _SUB)]
    while len(parts) > 1:
        parts = [
            parts[i] + parts[i + 1] if i + 1 < len(parts) else parts[i]
            for i in range(0, len(parts), 2)
        ]
    return parts[0]


def _compiler_params():
    opts = dict(collective_id=0, vmem_limit_bytes=32 * 1024 * 1024)
    for name in ("disable_semaphore_checks", "disable_bounds_checks"):
        if hasattr(pltpu.CompilerParams, name):
            opts[name] = True
    return pltpu.CompilerParams(**opts)


def pallas_dist_mean_ax0_shard0_i_m2048_n1024_kernel(
x: jax.Array,
):
    m_per, n = x.shape
    head = 2 * _OFF_ROWS
    tail_rows = sum(_TAIL_A_ROWS)
    t0 = m_per - tail_rows
    n_a = n - _TAIL_COLS
    chunk_rows = [head, 512, 512, t0 - head - 1024 - 128, 128]
    assert min(chunk_rows) > 0 and all(r % _SUB == 0 for r in chunk_rows)
    assert sum(chunk_rows) == t0 and n % 128 == 0 and n_a > 0
    n_chunks = len(chunk_rows)
    offsets = [sum(chunk_rows[:c]) for c in range(n_chunks)]
    a_offsets = [t0 + sum(_TAIL_A_ROWS[:i]) for i in range(len(_TAIL_A_ROWS))]
    n_loads = n_chunks + len(_TAIL_A_ROWS) + 1
    inv_count = 1.0 / float(_N_DEV * m_per)

    msg_diag_a = (2, 0, n_a, 0)
    msg_diag_b = (2, n_a, _TAIL_COLS, 1)
    msg_right = (1, 0, n, 2)
    msg_left = (3, 0, n, 3)

    def body(x_hbm, out_ref, buf, obuf, comm,
             load_sems, send_sems, recv_sems, osend_sems, orecv_sem):

        def load(r0, rows, c0, cols, slot):
            return pltpu.make_async_copy(
                x_hbm.at[pl.ds(r0, rows), pl.ds(c0, cols)],
                buf.at[pl.ds(r0, rows), pl.ds(c0, cols)],
                load_sems.at[slot],
            )

        loads = [load(offsets[c], chunk_rows[c], 0, n, c) for c in range(n_chunks)]
        tails_a = [
            load(a_offsets[i], _TAIL_A_ROWS[i], 0, n_a, n_chunks + i)
            for i in range(len(_TAIL_A_ROWS))
        ]
        tail_b = load(t0, tail_rows, n_a, _TAIL_COLS, n_loads - 1)

        loads[1].start()
        my = lax.axis_index("i")

        @pl.when(my != _LATE)
        def _():
            loads[0].start()

        for cp in loads[2:] + tails_a + [tail_b]:
            cp.start()

        barrier = pltpu.get_barrier_semaphore()
        for d in range(1, _N_DEV):
            pl.semaphore_signal(
                barrier, inc=1, device_id=((my + d) % _N_DEV,), device_id_type=_MESH
            )
        pl.semaphore_wait(barrier, _N_DEV - 1)

        def offload(j):
            return pltpu.make_async_remote_copy(
                src_ref=x_hbm.at[pl.ds(j * _OFF_ROWS, _OFF_ROWS)],
                dst_ref=obuf,
                send_sem=osend_sems.at[j],
                recv_sem=orecv_sem,
                device_id=((_LATE + (1 if j else _N_DEV - 1)) % _N_DEV,),
                device_id_type=_MESH,
            )

        @pl.when(my == _LATE)
        def _():
            offload(0).start()
            offload(1).start()

        def zeros():
            return jnp.zeros((_SUB, n), jnp.float32)

        def chunk_sum(c):
            loads[c].wait()
            return _colsum8(buf[pl.ds(offsets[c], chunk_rows[c]), :])

        def shipped_sum():
            offload(0).wait_recv()
            return _colsum8(obuf[...])

        acc = chunk_sum(1)
        acc = acc + lax.cond(my != _LATE, lambda: chunk_sum(0), zeros)
        for c in range(2, n_chunks):
            acc = acc + chunk_sum(c)
        acc = acc + lax.cond((my % 2) != (_LATE % 2), shipped_sum, zeros)

        def message(spec, owner):
            dist, c0, width, slot = spec
            part = comm.at[owner, :, pl.ds(c0, width)]
            return pltpu.make_async_remote_copy(
                src_ref=part,
                dst_ref=part,
                send_sem=send_sems.at[slot],
                recv_sem=recv_sems.at[slot],
                device_id=((my + dist) % _N_DEV,),
                device_id_type=_MESH,
            )

        a = acc[:, :n_a]
        for i, cp in enumerate(tails_a):
            cp.wait()
            a = a + _colsum8(buf[pl.ds(a_offsets[i], _TAIL_A_ROWS[i]), pl.ds(0, n_a)])
        comm[my, :, pl.ds(0, n_a)] = jnp.sum(a, axis=0, keepdims=True)
        message(msg_diag_a, my).start()

        tail_b.wait()
        b = acc[:, n_a:] + _treesum8(buf[pl.ds(t0, tail_rows), pl.ds(n_a, _TAIL_COLS)])
        comm[my, :, pl.ds(n_a, _TAIL_COLS)] = jnp.sum(b, axis=0, keepdims=True)
        for spec in (msg_diag_b, msg_right, msg_left):
            message(spec, my).start()

        for spec in (msg_diag_a, msg_diag_b, msg_right, msg_left):
            message(spec, my).wait_send()

        @pl.when(my == _LATE)
        def _():
            offload(0).wait_send()
            offload(1).wait_send()

        for spec in (msg_right, msg_left, msg_diag_a, msg_diag_b):
            sender = (my + _N_DEV - spec[0]) % _N_DEV
            message(spec, sender).wait_recv()

        total = (comm[0] + comm[1]) + (comm[2] + comm[3])
        out_ref[...] = total * inv_count

    return pl.pallas_call(
        body,
        out_shape=jax.ShapeDtypeStruct((1, n), jnp.float32),
        in_specs=[pl.BlockSpec(memory_space=pl.ANY)],
        out_specs=pl.BlockSpec(memory_space=pltpu.VMEM),
        scratch_shapes=[
            pltpu.VMEM((m_per, n), jnp.float32),
            pltpu.VMEM((_OFF_ROWS, n), jnp.float32),
            pltpu.VMEM((_N_DEV, 1, n), jnp.float32),
            pltpu.SemaphoreType.DMA((n_loads,)),
            pltpu.SemaphoreType.DMA((4,)),
            pltpu.SemaphoreType.DMA((4,)),
            pltpu.SemaphoreType.DMA((2,)),
            pltpu.SemaphoreType.DMA,
        ],
        compiler_params=_compiler_params(),
    )(x)
```
